```python
import numpy as np

kernel_name = "dist_sparse_attn_blocksparse_qseq_b2_sq256_skv256_hq4_dh64"

def setup_inputs():
    x = np.random.randn(2, 1024, 512).astype(np.float32)
    Wq = np.random.randn(512, 1024).astype(np.float32) * 0.02
    K_ext = np.random.randn(2, 256, 16, 64).astype(np.float32)
    V_ext = np.random.randn(2, 256, 16, 64).astype(np.float32)
    Wo = np.random.randn(1024, 512).astype(np.float32) * 0.02
    return {"x": x, "Wq": Wq, "K_ext": K_ext, "V_ext": V_ext, "Wo": Wo}

def reference(x, Wq, K_ext, V_ext, Wo):
    B, Sq, Skv, Hq, Dh = 2, 1024, 256, 16, 64
    Q = (x @ Wq).reshape(B, Sq, Hq, Dh)
    qb = (np.arange(Sq) // 64)[:, None]
    kb = (np.arange(Skv) // 64)[None, :]
    mask = (qb == kb) | (kb == 0) | ((qb + kb) % 3 == 0)
    scores = np.einsum('bihd,bjhd->bhij', Q, K_ext).astype(np.float32) * 0.125
    scores = np.where(mask[None, None, :, :], scores, -1e9)
    scores_max = scores.max(axis=-1, keepdims=True)
    w = np.exp(scores - scores_max)
    row_keep = mask.any(axis=1)
    w_sum = np.where(row_keep[None, None, :, None], w.sum(axis=-1, keepdims=True), 1.0)
    w = w / w_sum
    w = np.where(row_keep[None, None, :, None], w, 0.0)
    ctx = np.einsum('bhij,bjhd->bihd', w, V_ext).reshape(B, Sq, Hq * Dh)
    return ctx @ Wo
```

```python
import contextlib
import math

import jax
import jax.numpy as jnp
from jax import lax
from jax.experimental import pallas as pl
from jax.experimental.pallas import tpu as pltpu

N_DEV = 4
B, SQ, DM = 2, 256, 512
PAIR = 128
SKV = 256
BLK = 64
BF16 = jnp.bfloat16
F32 = jnp.float32
MESH = pl.DeviceIdType.MESH
ROW_ORDER = (0, 3, 1, 2)
QSCALE = 0.125 * math.log2(math.e)
NT = (((1,), (1,)), ((), ()))
U32 = jnp.uint32


def pack(v):
    return pltpu.bitcast(v.astype(BF16), U32)


def unpack(w):
    return pltpu.bitcast(w, BF16)


def make_kernel(out_dtype=F32, pieces=(64, 128, 320), asym_barrier=False, checks=False, scopes=False, flags=None):
    piece_off = [sum(pieces[:i]) for i in range(len(pieces))]
    NP = len(pieces)
    assert sum(pieces) == DM
    scope = jax.named_scope if scopes else (lambda name: contextlib.nullcontext())

    def body(x_hbm, wq_hbm, kt_hbm, vt_hbm, wo_hbm, o_ref,
             x_f32, wq_f32, wo_f32, k_f32, v_f32,
             x_bf, wq, wo, kz, vc, ctx, acc,
             ld_sem, kv_sem, snd, rcv, hello):
        me = lax.axis_index("i")
        right = (me + 1) % N_DEV
        left = (me + 3) % N_DEV
        diag = (me + 2) % N_DEV
        pair_of_slot = (2 * me, 2 * me + 1, 2 * left, 2 * right + 1,
                        2 * left + 1, 2 * right, 2 * diag, 2 * diag + 1)

        wq_ld = [pltpu.make_async_copy(wq_hbm.at[pl.ds(o, n)], wq_f32.at[pl.ds(o, n)], ld_sem.at[i])
                 for i, (o, n) in enumerate(zip(piece_off, pieces))]
        wo_ld = pltpu.make_async_copy(wo_hbm, wo_f32, ld_sem.at[NP])
        x_ld = pltpu.make_async_copy(x_hbm, x_f32, ld_sem.at[NP + 1])
        k_ld = [pltpu.make_async_copy(kt_hbm.at[:, pair_of_slot[s]], k_f32.at[s], kv_sem.at[0, s]) for s in range(8)]
        v_ld = [pltpu.make_async_copy(vt_hbm.at[:, pair_of_slot[s]], v_f32.at[s], kv_sem.at[1, s]) for s in range(8)]
        for c in wq_ld:
            c.start()

        barrier = pltpu.get_barrier_semaphore()
        odd = me % 2 == 1
        if not asym_barrier:
            for n in (left, right):
                pl.semaphore_signal(barrier, inc=1, device_id=(n,), device_id_type=MESH)
        else:
            @pl.when(me != 2)
            def _():
                for n in (left, right):
                    pl.semaphore_signal(barrier, inc=1, device_id=(n,), device_id_type=MESH)

        def remote(src, dst, k, to_right):
            d = 0 if to_right else 1
            return pltpu.make_async_remote_copy(
                src, dst, snd.at[d, k], rcv.at[d, k],
                device_id=(right if to_right else left,), device_id_type=MESH)

        def q_piece(src_slot, dst_slot, i, to_right):
            rows = pl.ds(piece_off[i] // 2, pieces[i] // 2)
            return remote(wq.at[src_slot, rows], wq.at[dst_slot, rows], i, to_right)

        q1 = [[q_piece(0, 2, i, True) for i in range(NP)], [q_piece(1, 3, i, False) for i in range(NP)]]
        q2 = [remote(wq.at[1], wq.at[4], NP, True), remote(wq.at[0], wq.at[5], NP, False)]
        qf = [remote(wq.at[2], wq.at[6], NP + 1, True), remote(wq.at[3], wq.at[7], NP + 1, False)]
        o1 = [remote(wo.at[0], wo.at[2], NP + 2, True), remote(wo.at[1], wo.at[3], NP + 2, False)]
        o2 = [remote(wo.at[1], wo.at[4], NP + 3, True), remote(wo.at[0], wo.at[5], NP + 3, False)]
        of = [[remote(wo.at[2, j], wo.at[6, j], NP + 4 + j, True) for j in range(4)],
              [remote(wo.at[3, j], wo.at[7, j], NP + 4 + j, False) for j in range(4)]]

        def cast_wq(i):
            wq_ld[i].wait()
            rows = pl.ds(piece_off[i], pieces[i])
            half = pl.ds(piece_off[i] // 2, pieces[i] // 2)
            wq[0, half] = pack(wq_f32[rows, 0:PAIR])
            wq[1, half] = pack(wq_f32[rows, PAIR:2 * PAIR])

        def first_loads():
            x_ld.start()
            k_ld[0].start()
            k_ld[1].start()

        if not asym_barrier:
            for i in range(NP):
                cast_wq(i)
            first_loads()
            pl.semaphore_wait(barrier, 2)
            for i in range(NP):
                q1[0][i].start()
                q1[1][i].start()
            q2[0].start()
            q2[1].start()
        else:
            cast_wq(0)

            @pl.when(odd)
            def _():
                pl.semaphore_wait(barrier, 1)

            for i in range(NP):
                if i:
                    cast_wq(i)

                @pl.when(me == 3)
                def _():
                    q1[0][i].start()

                @pl.when(me == 1)
                def _():
                    q1[1][i].start()

            @pl.when(me == 3)
            def _():
                q2[0].start()

            @pl.when(me == 1)
            def _():
                q2[1].start()

            first_loads()

            @pl.when(jnp.logical_not(odd))
            def _():
                pl.semaphore_wait(barrier, 2)

            @pl.when(me == 2)
            def _():
                for n in (left, right):
                    pl.semaphore_signal(hello, inc=1, device_id=(n,), device_id_type=MESH)

            @pl.when(odd)
            def _():
                pl.semaphore_wait(hello, 1)

            @pl.when(me != 3)
            def _():
                for i in range(NP):
                    q1[0][i].start()
                q2[0].start()

            @pl.when(me != 1)
            def _():
                for i in range(NP):
                    q1[1][i].start()
                q2[1].start()

        lane = lax.broadcasted_iota(jnp.int32, (BLK, 128), 1)
        low = lane < BLK

        def build_k(s):
            k_ld[s].wait()
            for b in range(B):
                kz[s, b] = pltpu.bitcast(k_f32[s, b].astype(BF16).T, U32)

        def build_v(s):
            v_ld[s].wait()
            for b in range(B):
                t0 = pack(v_f32[s, b, :, 0:128])
                t1 = pack(v_f32[s, b, :, 128:256])
                upper = (t1, pltpu.roll(t1, BLK, 1), t0)
                for c in range(3):
                    vc[s, b, (c + 2 * me) % 3] = t0 if c == 2 else jnp.where(low, t0, upper[c])

        HB = BLK // 2
        kb = [pl.multiple_of((3 - (me + g) % 3) * HB, HB) for g in range(3)]
        lane_blk = lax.broadcasted_iota(jnp.int32, (BLK, 256), 1) % 128
        keep_b = jnp.logical_or(lane_blk < BLK, me == 0)
        keep_c = jnp.logical_or(lane_blk >= BLK, me == 0)
        zeros = jnp.zeros((HB, 256), U32)

        def inv(l):
            r = pl.reciprocal(l, approx=True)
            return r * (2.0 - l * r)

        def q_proj(s):
            xq = unpack(jnp.concatenate([x_bf[k] for k in range(4)], axis=1))
            return pack(jnp.dot(xq, unpack(wq[s]), preferred_element_type=F32))

        def softmax(sc):
            p = jnp.exp2(sc - jnp.max(sc, axis=0, keepdims=True))
            return pack(p), inv(jnp.sum(p, axis=0, keepdims=True))

        def attend(s, q=None):
            if q is None:
                q = q_proj(s)
            scores = {}
            for g in range(2):
                for b in range(B):
                    qg = q[(2 * b + g) * BLK:(2 * b + g + 1) * BLK]
                    qz = jnp.concatenate([jnp.where(low, qg, 0), jnp.where(low, 0, qg)], axis=0)
                    blocks = (0, kb[0]) if g == 0 else (0, kb[1], kb[2])
                    k = jnp.concatenate([kz[s, b, pl.ds(r, HB)] for r in blocks], axis=0)
                    scores[g, b] = lax.dot_general(unpack(k), unpack(qz), NT, preferred_element_type=F32)
            probs = {}
            for b in range(B):
                probs[0, b] = softmax(scores[0, b])
            for b in range(B):
                sc = scores[1, b]
                p, r = softmax(jnp.concatenate([
                    sc[:BLK],
                    jnp.where(keep_b, sc[BLK:2 * BLK], -jnp.inf),
                    jnp.where(keep_c, sc[2 * BLK:], -jnp.inf)], axis=0))
                probs[1, b] = jnp.concatenate([p[:2 * HB], zeros, p[2 * HB:]], axis=0), r
            for g in range(2):
                for b in range(B):
                    p, r = probs[g, b]
                    cs = []
                    for h in range(2):
                        rows = pl.ds(h * HB, HB)
                        v = vc[s, b, 0, rows] if g == 0 else jnp.concatenate([vc[s, b, 1, rows], vc[s, b, 2, rows]], axis=1)
                        cols = slice(h * 128, (h + 1) * 128)
                        c = jnp.dot(unpack(v), unpack(p[:, cols]), preferred_element_type=F32)
                        cs.append(c * r[:, cols])
                    c = jnp.concatenate(cs, axis=0).astype(BF16).T
                    ctx[s, pl.ds((2 * b + g) * BLK, BLK)] = pltpu.bitcast(c, U32)

        def wo_mat(s):
            return unpack(jnp.concatenate(
                [jnp.concatenate([wo[s + h, j] for j in range(4)], axis=1) for h in range(2)], axis=0))

        def project(s):
            c = unpack(jnp.concatenate([ctx[s], ctx[s + 1]], axis=1))
            return jnp.dot(c, wo_mat(s), preferred_element_type=F32)

        with scope("x"):
            x_ld.wait()
            v_ld[0].start()
            v_ld[1].start()
            wo_ld.start()
            for b in range(B):
                for t, j in enumerate(ROW_ORDER):
                    xs = pack(x_f32[b, pl.ds(j * BLK, BLK)] * QSCALE)
                    for k in range(4):
                        x_bf[k, pl.ds((b * SQ + t * BLK) // 2, BLK // 2)] = xs[:, k * 128:(k + 1) * 128]
        with scope("build01"):
            build_k(0)
            build_k(1)
            build_v(0)
            build_v(1)
            wo_ld.wait()
            for s in (2, 3):
                k_ld[s].start()
                v_ld[s].start()
            for h in range(2):
                for j in range(4):
                    wo[h, j] = pack(wo_f32[h * PAIR:(h + 1) * PAIR, j * 128:(j + 1) * 128])
        with scope("att0"):
            attend(0)
        with scope("fwd1"):
            for d in range(2):
                for i in range(NP):
                    q1[d][i].wait_recv()
                qf[d].start()
                o1[d].start()
                o2[d].start()
        with scope("build23"):
            for s in (2, 3):
                build_k(s)
                build_v(s)
            for s in (4, 5):
                k_ld[s].start()
                v_ld[s].start()
        with scope("att1"):
            attend(1)
        with scope("att23"):
            for s in (2, 3):
                attend(s)
        with scope("build45"):
            for s in (4, 5):
                build_k(s)
                build_v(s)
            for s in (6, 7):
                k_ld[s].start()
                v_ld[s].start()
        with scope("wait_q2"):
            for d in range(2):
                q2[d].wait_recv()
        with scope("att45"):
            for s in (4, 5):
                attend(s)
        with scope("build67"):
            for s in (6, 7):
                build_k(s)
                build_v(s)
        with scope("wait_qf"):
            for d in range(2):
                qf[d].wait_recv()
        with scope("att67"):
            for s in (6, 7):
                attend(s)
        with scope("fwd2"):
            for d in range(2):
                o1[d].wait_recv()
                for j in range(4):
                    of[d][j].start()
        with scope("proj0"):
            acc[...] = project(0)
        with scope("proj2"):
            acc[...] += project(2)
        with scope("wait_o2"):
            for d in range(2):
                o2[d].wait_recv()
        with scope("proj4"):
            acc[...] += project(4)

        for j in range(4):
            with scope(f"wait_of{j}"):
                for d in range(2):
                    of[d][j].wait_recv()
            with scope(f"fin{j}"):
                cols = slice(j * 128, (j + 1) * 128)
                w = unpack(jnp.concatenate([wo[6, j], wo[7, j]], axis=0))
                c = unpack(jnp.concatenate([ctx[6], ctx[7]], axis=1))
                res = acc[:, cols] + jnp.dot(c, w, preferred_element_type=F32)
                for b in range(B):
                    for t, jb in enumerate(ROW_ORDER):
                        r0 = b * SQ + t * BLK
                        o_ref[b, pl.ds(jb * BLK, BLK), cols] = res[r0:r0 + BLK].astype(out_dtype)

        with scope("drain"):
            for d in range(2):
                for c in q1[d] + [q2[d], qf[d], o1[d], o2[d]] + of[d]:
                    c.wait_send()

    def kernel(x, Wq, K_ext, V_ext, Wo):
        kt = jnp.transpose(K_ext, (0, 2, 3, 1)).reshape(B, 8, PAIR, SKV)
        vt = jnp.transpose(V_ext, (0, 2, 3, 1)).reshape(B, 8, PAIR, SKV)
        hbm = pl.BlockSpec(memory_space=pltpu.HBM)
        return pl.pallas_call(
            body,
            out_shape=jax.ShapeDtypeStruct((B, SQ, DM), out_dtype),
            in_specs=[hbm] * 5,
            out_specs=pl.BlockSpec(memory_space=pltpu.VMEM),
            scratch_shapes=[
                pltpu.VMEM((B, SQ, DM), F32),
                pltpu.VMEM((DM, 2 * PAIR), F32),
                pltpu.VMEM((2 * PAIR, DM), F32),
                pltpu.VMEM((8, B, PAIR, SKV), F32),
                pltpu.VMEM((8, B, PAIR, SKV), F32),
                pltpu.VMEM((4, B * SQ // 2, 128), U32),
                pltpu.VMEM((8, DM // 2, PAIR), U32),
                pltpu.VMEM((8, 4, PAIR // 2, 128), U32),
                pltpu.VMEM((8, B, SKV // 2, PAIR), U32),
                pltpu.VMEM((8, B, 3, PAIR // 2, 128), U32),
                pltpu.VMEM((8, B * SQ // 2, PAIR), U32),
                pltpu.VMEM((B * SQ, DM), F32),
                pltpu.SemaphoreType.DMA((NP + 2,)),
                pltpu.SemaphoreType.DMA((2, 8)),
                pltpu.SemaphoreType.DMA((2, NP + 8)),
                pltpu.SemaphoreType.DMA((2, NP + 8)),
                pltpu.SemaphoreType.REGULAR,
            ],
            compiler_params=pltpu.CompilerParams(
                collective_id=0, vmem_limit_bytes=48 * 1024 * 1024, flags=flags,
                disable_bounds_checks=not checks, disable_semaphore_checks=not checks),
        )(x, Wq, kt, vt, Wo)

    return kernel


_kernel = make_kernel(out_dtype=F32, asym_barrier=True)


def pallas_dist_sparse_attn_blocksparse_qseq_b2_sq256_skv256_hq4_dh64_kernel(x, Wq, K_ext, V_ext, Wo):
    return _kernel(x, Wq, K_ext, V_ext, Wo)
```

```python
import math

import jax
import jax.numpy as jnp
from jax import lax
from jax.experimental import pallas as pl
from jax.experimental.pallas import tpu as pltpu

B, SQ, SKV, DM = 2, 256, 256, 512
BLK = 64
PAIR = 2 * BLK
SLOTS = 8
SCALE = 0.125 * math.log2(math.e)
ROW_ORDER = (0, 3, 1, 2)

BF16, F32, I32 = jnp.bfloat16, jnp.float32, jnp.int32
MESH = pl.DeviceIdType.MESH
NT = (((1,), (1,)), ((), ()))

ROUTE = {
    "first": ((0, 2), (1, 3)),
    "second": ((1, 4), (0, 5)),
    "relay": ((2, 6), (3, 7)),
}
WQ_GROUPS = (8, 24)
WO_PARTS = ((0, 4), (4, 6), (6, 7), (7, 8))

EXPONENT = 0x7F800000
HIGH = 0x78007800
MISFIT = 1 << 16


def to_words(v):
    return pltpu.bitcast(v.astype(BF16), I32)


def to_bf16(w):
    return pltpu.bitcast(w, BF16)


def as_f32(w):
    return pltpu.bitcast(w, F32)


def over_sublanes(reduce, v):
    return jnp.broadcast_to(reduce(v, axis=0, keepdims=True), (8, 128))


def message_rows(vregs):
    return 6 * vregs + 2


def encode(w, msg):
    n = w.shape[0] // 8
    exponents = jnp.maximum(as_f32(w & EXPONENT), as_f32((w << 16) & EXPONENT))
    top = pltpu.bitcast(over_sublanes(jnp.max, exponents), I32)
    base = jnp.maximum(top - (15 << 23), 0)
    both = base | (base >> 16)

    row = lax.broadcasted_iota(I32, (8, 128), 0) | (1 << 23)
    total = jnp.zeros((8, 128), I32)
    count = largest = jnp.zeros((8, 128), F32)
    smallest = jnp.full((8, 128), jnp.inf, F32)
    t = []
    for i in range(n):
        t.append(w[8 * i:8 * i + 8] - both)
        high = t[i] & HIGH
        listed = high != 0
        entry = high | (row + 8 * i)
        total = total + jnp.where(listed, entry, 0)
        largest = jnp.maximum(largest, jnp.where(listed, as_f32(entry), 0.0))
        smallest = jnp.minimum(smallest, jnp.where(listed, as_f32(entry), jnp.inf))
        count = count + jnp.where(listed, 1.0, 0.0)

    body = []
    for i in range(0, n, 4):
        d = t[i + 3]
        body += [
            (t[i] & ~HIGH) | ((d << 11) & HIGH),
            (t[i + 1] & ~HIGH) | ((d << 7) & HIGH),
            (t[i + 2] & ~HIGH) | ((d << 3) & 0x38003800) | ((d >> 1) & 0x40004000),
        ]

    count = over_sublanes(jnp.sum, count)
    largest = pltpu.bitcast(over_sublanes(jnp.max, largest), I32)
    smallest = pltpu.bitcast(over_sublanes(jnp.min, smallest), I32)
    middle = over_sublanes(jnp.sum, total) - largest - smallest

    def short(entry):
        return ((entry >> 15) & 0xF000) | ((entry >> 3) & 0x0F00) | (entry & 0xFF)

    second = short(jnp.where(count >= 2.0, smallest, 0))
    third = short(jnp.where(count == 3.0, middle, 0))
    msg[pl.ds(0, 6 * n)] = jnp.concatenate(body, axis=0)
    msg[pl.ds(6 * n, 1)] = (base | jnp.where(count > 3.0, MISFIT, 0) | third)[0:1]
    msg[pl.ds(6 * n + 1, 1)] = ((short(largest) << 16) | second)[0:1]


def decode(msg, vregs=None):
    header = msg.shape[0] - 8
    if vregs is None:
        vregs = range(header // 6)
    head = jnp.broadcast_to(msg[pl.ds(header, 1)], (8, 128))
    more = jnp.broadcast_to(msg[pl.ds(header + 1, 1)], (8, 128))
    base = head & EXPONENT
    both = base | (base >> 16)
    row = lax.broadcasted_iota(I32, (8, 128), 0)
    entries = [
        ((z & 0xFF) - row, both + (((z & 0xF000) << 15) | ((z & 0x0F00) << 3)))
        for z in (head, more, more >> 16)
    ]
    out = []
    for i in vregs:
        first = 24 * (i // 4)
        if i % 4 < 3:
            t = msg[pl.ds(first + 8 * (i % 4), 8)] & ~HIGH
        else:
            a, b, c = (msg[pl.ds(first + 8 * k, 8)] for k in range(3))
            t = (((a & HIGH) >> 11) | ((b & HIGH) >> 7)
                 | ((c & 0x38003800) >> 3) | ((c & 0x40004000) << 1))
        offset = both
        for place, value in entries:
            offset = jnp.where(place == 8 * i, value, offset)
        out.append(t + offset)
    return jnp.concatenate(out, axis=0)


def _body(x_hbm, wq_hbm, kt_hbm, vt_hbm, wo_hbm, out_ref,
          x_f32, wq_f32, wo_f32, k_f32, v_f32,
          x_w, wq_w, wo_w, wq_msg0, wq_msg1, wo_msg, k_w, v_w, ctx_w, acc,
          load_sem, send_sem, recv_sem, plain_send_sem, plain_recv_sem, entered_sem):
    me = lax.axis_index("i")
    first = jnp.where(me == 1, 1, 0)
    second = 1 - first

    def wq_load(h, g):
        rows = pl.ds(16 * WQ_GROUPS[0] * g, 16 * WQ_GROUPS[g])
        cols = pl.ds(pl.multiple_of(h * PAIR, PAIR), PAIR)
        return pltpu.make_async_copy(wq_hbm.at[rows, cols], wq_f32.at[h, rows], load_sem.at[2 * h + g])

    wq_load(first, 0).start()

    right, diag, left = (me + 1) & 3, (me + 2) & 3, (me + 3) & 3
    neighbour = (right, left)
    wq_msg = (wq_msg0, wq_msg1)

    barrier = pltpu.get_barrier_semaphore()
    odd = (me & 1) == 1

    @pl.when(me != 2)
    def _():
        for n in neighbour:
            pl.semaphore_signal(barrier, inc=1, device_id=(n,), device_id_type=MESH)

    pair_in_slot = (2 * me, 2 * me + 1, 2 * left, 2 * right + 1,
                    2 * left + 1, 2 * right, 2 * diag, 2 * diag + 1)
    x_load = pltpu.make_async_copy(x_hbm, x_f32, load_sem.at[4])
    wo_load = pltpu.make_async_copy(wo_hbm, wo_f32, load_sem.at[5])
    k_load = [pltpu.make_async_copy(kt_hbm.at[:, p], k_f32.at[s], load_sem.at[6 + 2 * s])
              for s, p in enumerate(pair_in_slot)]
    v_load = [pltpu.make_async_copy(vt_hbm.at[:, p], v_f32.at[s], load_sem.at[7 + 2 * s])
              for s, p in enumerate(pair_in_slot)]
    for copy in (wq_load(second, 0), wq_load(first, 1), wq_load(second, 1),
                 x_load, k_load[0], wo_load, v_load[0]):
        copy.start()
    for s in range(1, SLOTS):
        k_load[s].start()
        v_load[s].start()

    def remote(buf, stage, d, rows, sems, k):
        src, dst = ROUTE[stage][d]
        return pltpu.make_async_remote_copy(
            buf.at[src, rows], buf.at[dst, rows], sems[0].at[d, k], sems[1].at[d, k],
            device_id=(neighbour[d],), device_id_type=MESH)

    def quarters(lo, hi):
        return pl.ds(24 * lo, 24 * (hi - lo))

    half = WO_PARTS[0][1]
    wo_header = pl.ds(24 * 8, 2)
    wo_rows = {
        "first": (6, [wo_header, quarters(0, half), quarters(half, 8)]),
        "second": (9, [pl.ds(0, message_rows(32))]),
        "relay": (10, [wo_header] + [quarters(*part) for part in WO_PARTS]),
    }
    sems = (send_sem, recv_sem)
    wq_copy, wo_copy = {}, {}
    for n, stage in enumerate(ROUTE):
        for d in range(2):
            wq_copy[stage, d] = [
                remote(wq_msg[g], stage, d, pl.ds(0, message_rows(WQ_GROUPS[g])), sems, 2 * n + g)
                for g in range(2)]
            k, parts = wo_rows[stage]
            wo_copy[stage, d] = [remote(wo_msg, stage, d, rows, sems, k + i) for i, rows in enumerate(parts)]

    def start(*copies):
        for copy in copies:
            copy.start()

    def start_if(condition, *copies):
        pl.when(condition)(lambda: start(*copies))

    def wait_recv(*copies):
        for copy in copies:
            copy.wait_recv()

    def wait_send(*copies):
        for copy in copies:
            copy.wait_send()

    @pl.when(me == 2)
    def _():
        pl.semaphore_wait(barrier, 2)
        for n in neighbour:
            pl.semaphore_signal(entered_sem, inc=1, device_id=(n,), device_id_type=MESH)

    def pack_wq(h, g):
        wq_load(h, g).wait()
        w = to_words(wq_f32[h, pl.ds(16 * WQ_GROUPS[0] * g, 16 * WQ_GROUPS[g])])
        wq_w[h, pl.ds(8 * WQ_GROUPS[0] * g, 8 * WQ_GROUPS[g])] = w
        encode(w, wq_msg[g].at[h])

    ready = (jnp.logical_or(me == 3, me == 2), jnp.logical_or(me == 1, me == 2))
    pack_wq(first, 0)
    pl.when(odd)(lambda: pl.semaphore_wait(barrier, 1))
    for g in range(2):
        if g:
            pack_wq(first, g)
        start_if(ready[0], wq_copy["first", 0][g])
        start_if(me == 1, wq_copy["first", 1][g])
        pack_wq(second, g)
        start_if(me == 2, wq_copy["first", 1][g])
    for d in range(2):
        start_if(ready[d], *wq_copy["second", d])
    pl.when(me == 0)(lambda: pl.semaphore_wait(barrier, 2))
    pl.when(odd)(lambda: pl.semaphore_wait(entered_sem, 1))
    for d in range(2):
        start_if(jnp.logical_not(ready[d]), *wq_copy["first", d], *wq_copy["second", d])

    key_rows = [pl.multiple_of((3 - (me + g) % 3) * (BLK // 2), BLK // 2) for g in range(3)]
    column = lax.broadcasted_iota(I32, (BLK, 2 * PAIR), 1) % PAIR
    sees_block_1 = jnp.logical_or(column < BLK, me == 0)
    sees_block_2 = jnp.logical_or(column >= BLK, me == 0)

    def low_lanes(rows):
        return lax.broadcasted_iota(I32, (rows, PAIR), 1) < BLK

    def prepare_keys(s):
        for b in range(B):
            k_w[s, b] = pltpu.bitcast(k_f32[s, b].astype(BF16).T, I32)

    def prepare_values(s):
        for b in range(B):
            front = to_words(v_f32[s, b, :, 0:PAIR])
            back = to_words(v_f32[s, b, :, PAIR:SKV])
            tiles = (jnp.where(low_lanes(BLK), front, back),
                     jnp.where(low_lanes(BLK), front, pltpu.roll(back, BLK, 1)),
                     front)
            for residue, tile in enumerate(tiles):
                v_w[s, b, (residue + 2 * me) % 3] = tile

    def queries(w):
        x = to_bf16(jnp.concatenate([x_w[k] for k in range(DM // 128)], axis=1))
        return jnp.dot(x, to_bf16(w), preferred_element_type=F32)

    def scores(s, q):
        out = {}
        for part in range(2):
            for b in range(B):
                rows = q[(2 * b + part) * PAIR:(2 * b + part + 1) * PAIR]
                per_head = jnp.concatenate(
                    [jnp.where(low_lanes(PAIR), rows, 0.0), jnp.where(low_lanes(PAIR), 0.0, rows)], axis=0)
                blocks = (0, key_rows[0]) if part == 0 else (0, key_rows[1], key_rows[2])
                k = jnp.concatenate([k_w[s, b, pl.ds(r, BLK // 2)] for r in blocks], axis=0)
                out[part, b] = lax.dot_general(to_bf16(k), per_head.astype(BF16), NT, preferred_element_type=F32)
        return out

    def softmax(sc):
        p = jnp.exp2(sc - jnp.max(sc, axis=0, keepdims=True))
        total = jnp.sum(p, axis=0, keepdims=True)
        r = pl.reciprocal(total, approx=True)
        return p, r * (2.0 - total * r)

    def weighted_values(s, sc):
        probs = {(0, b): softmax(sc[0, b]) for b in range(B)}
        for b in range(B):
            p, r = softmax(jnp.concatenate([
                sc[1, b][:BLK],
                jnp.where(sees_block_1, sc[1, b][BLK:2 * BLK], -jnp.inf),
                jnp.where(sees_block_2, sc[1, b][2 * BLK:], -jnp.inf)], axis=0))
            probs[1, b] = jnp.concatenate([p[:2 * BLK], jnp.zeros((BLK, 2 * PAIR), F32), p[2 * BLK:]], axis=0), r
        out = {}
        for part in range(2):
            for b in range(B):
                p, r = probs[part, b]
                out[part, b] = []
                for h in range(2):
                    rows = pl.ds(h * BLK // 2, BLK // 2)
                    if part == 0:
                        v = v_w[s, b, 0, rows]
                    else:
                        v = jnp.concatenate([v_w[s, b, 1, rows], v_w[s, b, 2, rows]], axis=1)
                    cols = slice(h * PAIR, (h + 1) * PAIR)
                    pv = jnp.dot(to_bf16(v), p[:, cols].astype(BF16), preferred_element_type=F32)
                    out[part, b].append((pv, r[:, cols]))
        return out

    def store_context(s, heads):
        for part in range(2):
            for b in range(B):
                c = jnp.concatenate([pv * r for pv, r in heads[part, b]], axis=0).astype(BF16).T
                ctx_w[s, pl.ds((2 * b + part) * BLK, BLK)] = pltpu.bitcast(c, I32)

    def project(s, words):
        c = jnp.concatenate([ctx_w[s], ctx_w[s + 1]], axis=1)
        w = jnp.concatenate(
            [jnp.concatenate([w[r:r + BLK] for r in range(0, w.shape[0], BLK)], axis=1) for w in words], axis=0)
        return jnp.dot(to_bf16(c), to_bf16(w), preferred_element_type=F32)

    def received_wq(s):
        return jnp.concatenate([decode(msg.at[s]) for msg in wq_msg], axis=0)

    def received_wo(s, lo, hi):
        return decode(wo_msg.at[s], range(4 * lo, 4 * hi))

    def write_out(row, cols, value):
        for t in range(value.shape[0] // BLK):
            b, place = divmod(row // BLK + t, SQ // BLK)
            out_ref[b, pl.ds(ROW_ORDER[place] * BLK, BLK), cols] = value[t * BLK:(t + 1) * BLK].astype(out_ref.dtype)

    x_load.wait()
    for b in range(B):
        for place, block in enumerate(ROW_ORDER):
            w = to_words(x_f32[b, pl.ds(block * BLK, BLK)] * SCALE)
            for k in range(DM // 128):
                x_w[k, pl.ds((b * SQ + place * BLK) // 2, BLK // 2)] = w[:, k * 128:(k + 1) * 128]
    q = queries(wq_w[0])

    wo_load.wait()
    for h in range(2):
        w = jnp.concatenate(
            [to_words(wo_f32[h * PAIR:(h + 1) * PAIR, j * 128:(j + 1) * 128]) for j in range(DM // 128)], axis=0)
        wo_w[h] = w
        encode(w, wo_msg.at[h])
    for d in range(2):
        start(*wo_copy["first", d][:2])
    k_load[0].wait()
    prepare_keys(0)

    heads = None
    for s in range(SLOTS):
        if s == 1:
            for d in range(2):
                wait_recv(*wq_copy["first", d])
                start(*wq_copy["relay", d], *wo_copy["first", d][2:], *wo_copy["second", d])
        if s == 3:
            for d in range(2):
                wait_recv(*wq_copy["second", d])
        if s == 6:
            for d in range(2):
                wait_recv(*wo_copy["first", d][:2])
                start(*wo_copy["relay", d][:2])
            update = project(2, [received_wo(z, 0, half) for z in (2, 3)])
            store_context(5, heads)
            heads = None
            acc[:, 0:BLK * half] += update
            for d in range(2):
                wait_recv(*wq_copy["relay", d])
            q = queries(received_wq(6))
            for d in range(2):
                wait_recv(*wo_copy["first", d][2:])
                start(*wo_copy["relay", d][2:])
        v_load[s].wait()
        if s + 1 < SLOTS:
            k_load[s + 1].wait()

        sc = scores(s, q)
        if s == 7:
            heads_6 = heads
        elif heads is not None:
            store_context(s - 1, heads)
        if s == 5:
            acc[...] = project(0, (wo_w[0], wo_w[1]))
        elif s == 7:
            acc[:, BLK * half:DM] += project(2, [received_wo(z, half, 8) for z in (2, 3)])
        else:
            q = queries(wq_w[1] if s == 0 else received_wq(s + 1))
        if s + 1 < SLOTS:
            prepare_keys(s + 1)
        prepare_values(s)
        heads = weighted_values(s, sc)

    for d in range(2):
        wait_send(*wq_copy["first", d], *wq_copy["second", d], *wq_copy["relay", d], *wo_copy["first", d])
        wait_recv(*wo_copy["second", d])
    update = project(4, [received_wo(z, 0, 8) for z in (4, 5)])
    for h in range(2):
        store_context(6 + h, {key: [heads_6[key][h], heads[key][h]] for key in heads})
    acc[...] += update

    def finish_output(lo, hi):
        for j in range(lo // 2, (hi + 1) // 2):
            cols = slice(j * 128, (j + 1) * 128)
            hs = [h for h in range(2) if lo <= 2 * j + h < hi]
            w = to_bf16(jnp.concatenate(
                [received_wo(z, 2 * j + h, 2 * j + h + 1) for h in hs for z in (6, 7)], axis=0))
            rows = B * SQ * len(hs) // 4
            for r in range(0, B * SQ, rows):
                c = jnp.concatenate([ctx_w[6 + h, pl.ds(r // 2, rows // 2)] for h in hs], axis=1)
                value = acc[pl.ds(r, rows), cols] + jnp.dot(to_bf16(c), w, preferred_element_type=F32)
                if hs[-1] == 0:
                    acc[pl.ds(r, rows), cols] = value
                else:
                    write_out(r, cols, value)

    for i, part in enumerate(WO_PARTS):
        for d in range(2):
            if i == len(WO_PARTS) - 1:
                wait_send(*wo_copy["second", d], *wo_copy["relay", d][:-1])
            wait_recv(*wo_copy["relay", d][(i + 1 if i else 0):i + 2])
        if i == 0:
            headers = jnp.zeros((1, 128), I32)
            for s in range(SLOTS):
                for msg in (*wq_msg, wo_msg):
                    headers = headers | msg[s, pl.ds(msg.shape[1] - 8, 1)]
            misfit = jnp.max(jnp.where((headers & MISFIT) != 0, 1.0, 0.0)) > 0.0
        finish_output(*part)
    for d in range(2):
        wait_send(wo_copy["relay", d][-1])

    @pl.when(misfit)
    def _():
        def plain(stage):
            k = 2 * list(ROUTE).index(stage)
            return [remote(buf, stage, d, slice(None), (plain_send_sem, plain_recv_sem), k + i)
                    for d in range(2) for i, buf in enumerate((wq_w, wo_w))]

        for copies in (plain("first") + plain("second"), plain("relay")):
            start(*copies)
            wait_send(*copies)
            wait_recv(*copies)

        def attend(s, carry):
            store_context(s, weighted_values(s, scores(s, queries(wq_w[s]))))
            return carry

        def add(i, carry):
            acc[...] += project(2 * i, (wo_w[2 * i], wo_w[2 * i + 1]))
            return carry

        lax.fori_loop(0, SLOTS, attend, 0)
        acc[...] = jnp.zeros(acc.shape, F32)
        lax.fori_loop(0, SLOTS // 2, add, 0)
        write_out(0, slice(None), acc[...])


def pallas_dist_sparse_attn_blocksparse_qseq_b2_sq256_skv256_hq4_dh64_kernel(
    x: jax.Array,
    Wq: jax.Array,
    K_ext: jax.Array,
    V_ext: jax.Array,
    Wo: jax.Array,
):
    kt = jnp.transpose(K_ext, (0, 2, 3, 1)).reshape(B, SLOTS, PAIR, SKV)
    vt = jnp.transpose(V_ext, (0, 2, 3, 1)).reshape(B, SLOTS, PAIR, SKV)
    return pl.pallas_call(
        _body,
        out_shape=jax.ShapeDtypeStruct((B, SQ, DM), BF16),
        in_specs=[pl.BlockSpec(memory_space=pltpu.HBM)] * 5,
        out_specs=pl.BlockSpec(memory_space=pltpu.VMEM),
        scratch_shapes=[
            pltpu.VMEM((B, SQ, DM), F32),
            pltpu.VMEM((2, DM, PAIR), F32),
            pltpu.VMEM((2 * PAIR, DM), F32),
            pltpu.VMEM((SLOTS, B, PAIR, SKV), F32),
            pltpu.VMEM((SLOTS, B, PAIR, SKV), F32),
            pltpu.VMEM((DM // 128, B * SQ // 2, 128), I32),
            pltpu.VMEM((SLOTS, DM // 2, PAIR), I32),
            pltpu.VMEM((SLOTS, DM // 2, 128), I32),
            pltpu.VMEM((SLOTS, 6 * WQ_GROUPS[0] + 8, 128), I32),
            pltpu.VMEM((SLOTS, 6 * WQ_GROUPS[1] + 8, 128), I32),
            pltpu.VMEM((SLOTS, 6 * 32 + 8, 128), I32),
            pltpu.VMEM((SLOTS, B, SKV // 2, PAIR), I32),
            pltpu.VMEM((SLOTS, B, 3, PAIR // 2, 128), I32),
            pltpu.VMEM((SLOTS, B * SQ // 2, PAIR), I32),
            pltpu.VMEM((B * SQ, DM), F32),
            pltpu.SemaphoreType.DMA((6 + 2 * SLOTS,)),
            pltpu.SemaphoreType.DMA((2, 11 + len(WO_PARTS))),
            pltpu.SemaphoreType.DMA((2, 11 + len(WO_PARTS))),
            pltpu.SemaphoreType.DMA((2, 6)),
            pltpu.SemaphoreType.DMA((2, 6)),
            pltpu.SemaphoreType.REGULAR,
        ],
        compiler_params=pltpu.CompilerParams(
            collective_id=0,
            vmem_limit_bytes=48 * 1024 * 1024,
            disable_bounds_checks=True,
            disable_semaphore_checks=True,
        ),
    )(x, Wq, kt, vt, Wo)
```

```python
import math

import jax
import jax.numpy as jnp
from jax import lax
from jax.experimental import pallas as pl
from jax.experimental.pallas import tpu as pltpu

B, SQ, SKV, DM = 2, 256, 256, 512
BLK = 64
PAIR = 2 * BLK
SLOTS = 8
SCALE = 0.125 * math.log2(math.e)
ROW_ORDER = (0, 3, 1, 2)

BF16, F32, I32 = jnp.bfloat16, jnp.float32, jnp.int32
MESH = pl.DeviceIdType.MESH
NT = (((1,), (1,)), ((), ()))

ROUTE = {
    "first": ((0, 2), (1, 3)),
    "second": ((1, 4), (0, 5)),
    "relay": ((2, 6), (3, 7)),
}
WQ_GROUPS = (8, 24)
WO_PARTS = ((0, 4), (4, 6), (6, 7), (7, 8))

EXPONENT = 0x7F800000
HIGH = 0x78007800
MISFIT = 1 << 16


def to_words(v):
    return pltpu.bitcast(v.astype(BF16), I32)


def to_bf16(w):
    return pltpu.bitcast(w, BF16)


def as_f32(w):
    return pltpu.bitcast(w, F32)


def over_sublanes(reduce, v):
    return jnp.broadcast_to(reduce(v, axis=0, keepdims=True), (8, 128))


def message_rows(vregs):
    return 6 * vregs + 2


def encode(w, msg):
    n = w.shape[0] // 8
    exponents = jnp.maximum(as_f32(w & EXPONENT), as_f32((w << 16) & EXPONENT))
    top = pltpu.bitcast(over_sublanes(jnp.max, exponents), I32)
    base = jnp.maximum(top - (15 << 23), 0)
    both = base | (base >> 16)

    row = lax.broadcasted_iota(I32, (8, 128), 0) | (1 << 23)
    total = jnp.zeros((8, 128), I32)
    count = largest = jnp.zeros((8, 128), F32)
    smallest = jnp.full((8, 128), jnp.inf, F32)
    t = []
    for i in range(n):
        t.append(w[8 * i:8 * i + 8] - both)
        high = t[i] & HIGH
        listed = high != 0
        entry = high | (row + 8 * i)
        total = total + jnp.where(listed, entry, 0)
        largest = jnp.maximum(largest, jnp.where(listed, as_f32(entry), 0.0))
        smallest = jnp.minimum(smallest, jnp.where(listed, as_f32(entry), jnp.inf))
        count = count + jnp.where(listed, 1.0, 0.0)

    body = []
    for i in range(0, n, 4):
        d = t[i + 3]
        body += [
            (t[i] & ~HIGH) | ((d << 11) & HIGH),
            (t[i + 1] & ~HIGH) | ((d << 7) & HIGH),
            (t[i + 2] & ~HIGH) | ((d << 3) & 0x38003800) | ((d >> 1) & 0x40004000),
        ]

    count = over_sublanes(jnp.sum, count)
    largest = pltpu.bitcast(over_sublanes(jnp.max, largest), I32)
    smallest = pltpu.bitcast(over_sublanes(jnp.min, smallest), I32)
    middle = over_sublanes(jnp.sum, total) - largest - smallest

    def short(entry):
        return ((entry >> 15) & 0xF000) | ((entry >> 3) & 0x0F00) | (entry & 0xFF)

    second = short(jnp.where(count >= 2.0, smallest, 0))
    third = short(jnp.where(count == 3.0, middle, 0))
    msg[pl.ds(0, 6 * n)] = jnp.concatenate(body, axis=0)
    msg[pl.ds(6 * n, 1)] = (base | jnp.where(count > 3.0, MISFIT, 0) | third)[0:1]
    msg[pl.ds(6 * n + 1, 1)] = ((short(largest) << 16) | second)[0:1]


def read_header(msg):
    header = msg.shape[0] - 8
    head = jnp.broadcast_to(msg[pl.ds(header, 1)], (8, 128))
    more = jnp.broadcast_to(msg[pl.ds(header + 1, 1)], (8, 128))
    base = head & EXPONENT
    both = base | (base >> 16)
    row = lax.broadcasted_iota(I32, (8, 128), 0)
    return both, [
        ((z & 0xFF) - row, both + (((z & 0xF000) << 15) | ((z & 0x0F00) << 3)))
        for z in (head, more, more >> 16)
    ]


def decode(msg, vregs=None, header=None):
    both, entries = header or read_header(msg)
    out = []
    for i in vregs or range((msg.shape[0] - 8) // 6):
        first = 24 * (i // 4)
        if i % 4 < 3:
            t = msg[pl.ds(first + 8 * (i % 4), 8)] & ~HIGH
        else:
            a, b, c = (msg[pl.ds(first + 8 * k, 8)] for k in range(3))
            t = (((a & HIGH) >> 11) | ((b & HIGH) >> 7)
                 | ((c & 0x38003800) >> 3) | ((c & 0x40004000) << 1))
        offset = both
        for place, value in entries:
            offset = jnp.where(place == 8 * i, value, offset)
        out.append(t + offset)
    return jnp.concatenate(out, axis=0)


def _body(x_hbm, wq_hbm, kt_hbm, vt_hbm, wo_hbm, out_ref,
          x_f32, wq_f32, wo_f32, k_f32, v_f32,
          x_w, wq_w, wo_w, wq_msg0, wq_msg1, wo_msg, k_w, v_w, ctx_w, acc,
          load_sem, send_sem, recv_sem, plain_send_sem, plain_recv_sem, entered_sem):
    me = lax.axis_index("i")
    first = jnp.where(me == 1, 1, 0)
    second = 1 - first

    def wq_load(h, g):
        rows = pl.ds(16 * WQ_GROUPS[0] * g, 16 * WQ_GROUPS[g])
        cols = pl.ds(pl.multiple_of(h * PAIR, PAIR), PAIR)
        return pltpu.make_async_copy(wq_hbm.at[rows, cols], wq_f32.at[h, rows], load_sem.at[2 * h + g])

    wq_load(first, 0).start()

    right, diag, left = (me + 1) & 3, (me + 2) & 3, (me + 3) & 3
    neighbour = (right, left)
    wq_msg = (wq_msg0, wq_msg1)

    barrier = pltpu.get_barrier_semaphore()
    odd = (me & 1) == 1

    @pl.when(me != 2)
    def _():
        for n in neighbour:
            pl.semaphore_signal(barrier, inc=1, device_id=(n,), device_id_type=MESH)

    pair_in_slot = (2 * me, 2 * me + 1, 2 * left, 2 * right + 1,
                    2 * left + 1, 2 * right, 2 * diag, 2 * diag + 1)
    x_load = pltpu.make_async_copy(x_hbm, x_f32, load_sem.at[4])
    wo_load = pltpu.make_async_copy(wo_hbm, wo_f32, load_sem.at[5])
    k_load = [pltpu.make_async_copy(kt_hbm.at[:, p], k_f32.at[s], load_sem.at[6 + 2 * s])
              for s, p in enumerate(pair_in_slot)]
    v_load = [pltpu.make_async_copy(vt_hbm.at[:, p], v_f32.at[s], load_sem.at[7 + 2 * s])
              for s, p in enumerate(pair_in_slot)]
    for copy in (wq_load(second, 0), wq_load(first, 1), wq_load(second, 1),
                 x_load, k_load[0], wo_load, v_load[0]):
        copy.start()
    for s in range(1, SLOTS):
        k_load[s].start()
        v_load[s].start()

    def remote(buf, stage, d, rows, sems, k):
        src, dst = ROUTE[stage][d]
        return pltpu.make_async_remote_copy(
            buf.at[src, rows], buf.at[dst, rows], sems[0].at[d, k], sems[1].at[d, k],
            device_id=(neighbour[d],), device_id_type=MESH)

    def quarters(lo, hi):
        return pl.ds(24 * lo, 24 * (hi - lo))

    half = WO_PARTS[0][1]
    wo_header = pl.ds(24 * 8, 2)
    wo_rows = {
        "first": (6, [wo_header, quarters(0, half), quarters(half, 8)]),
        "second": (9, [pl.ds(0, message_rows(32))]),
        "relay": (10, [wo_header] + [quarters(*part) for part in WO_PARTS]),
    }
    sems = (send_sem, recv_sem)
    wq_copy, wo_copy = {}, {}
    for n, stage in enumerate(ROUTE):
        for d in range(2):
            wq_copy[stage, d] = [
                remote(wq_msg[g], stage, d, pl.ds(0, message_rows(WQ_GROUPS[g])), sems, 2 * n + g)
                for g in range(2)]
            k, parts = wo_rows[stage]
            wo_copy[stage, d] = [remote(wo_msg, stage, d, rows, sems, k + i) for i, rows in enumerate(parts)]

    def start(*copies):
        for copy in copies:
            copy.start()

    def start_if(condition, *copies):
        pl.when(condition)(lambda: start(*copies))

    def wait_recv(*copies):
        for copy in copies:
            copy.wait_recv()

    def wait_send(*copies):
        for copy in copies:
            copy.wait_send()

    @pl.when(me == 2)
    def _():
        pl.semaphore_wait(barrier, 2)
        for n in neighbour:
            pl.semaphore_signal(entered_sem, inc=1, device_id=(n,), device_id_type=MESH)

    def pack_wq(h, g):
        wq_load(h, g).wait()
        w = to_words(wq_f32[h, pl.ds(16 * WQ_GROUPS[0] * g, 16 * WQ_GROUPS[g])])
        wq_w[h, pl.ds(8 * WQ_GROUPS[0] * g, 8 * WQ_GROUPS[g])] = w
        encode(w, wq_msg[g].at[h])

    ready = (jnp.logical_or(me == 3, me == 2), jnp.logical_or(me == 1, me == 2))
    pack_wq(first, 0)
    pl.when(odd)(lambda: pl.semaphore_wait(barrier, 1))
    for g in range(2):
        if g:
            pack_wq(first, g)
        start_if(ready[0], wq_copy["first", 0][g])
        start_if(me == 1, wq_copy["first", 1][g])
        pack_wq(second, g)
        start_if(me == 2, wq_copy["first", 1][g])
    for d in range(2):
        start_if(ready[d], *wq_copy["second", d])
    pl.when(me == 0)(lambda: pl.semaphore_wait(barrier, 2))
    pl.when(odd)(lambda: pl.semaphore_wait(entered_sem, 1))
    for d in range(2):
        start_if(jnp.logical_not(ready[d]), *wq_copy["first", d], *wq_copy["second", d])

    key_rows = [pl.multiple_of((3 - (me + g) % 3) * (BLK // 2), BLK // 2) for g in range(3)]
    column = lax.broadcasted_iota(I32, (BLK, 2 * PAIR), 1) % PAIR
    sees_block_1 = jnp.logical_or(column < BLK, me == 0)
    sees_block_2 = jnp.logical_or(column >= BLK, me == 0)

    def low_lanes(rows):
        return lax.broadcasted_iota(I32, (rows, PAIR), 1) < BLK

    def prepare_keys(s):
        for b in range(B):
            k_w[s, b] = pltpu.bitcast(k_f32[s, b].astype(BF16).T, I32)

    def prepare_values(s):
        for b in range(B):
            front = to_words(v_f32[s, b, :, 0:PAIR])
            back = to_words(v_f32[s, b, :, PAIR:SKV])
            tiles = (jnp.where(low_lanes(BLK), front, back),
                     jnp.where(low_lanes(BLK), front, pltpu.roll(back, BLK, 1)),
                     front)
            for residue, tile in enumerate(tiles):
                v_w[s, b, (residue + 2 * me) % 3] = tile

    def queries(w):
        x = to_bf16(jnp.concatenate([x_w[k] for k in range(DM // 128)], axis=1))
        return jnp.dot(x, to_bf16(w), preferred_element_type=F32)

    def scores(s, q):
        out = {}
        for part in range(2):
            for b in range(B):
                rows = q[(2 * b + part) * PAIR:(2 * b + part + 1) * PAIR]
                per_head = jnp.concatenate(
                    [jnp.where(low_lanes(PAIR), rows, 0.0), jnp.where(low_lanes(PAIR), 0.0, rows)], axis=0)
                blocks = (0, key_rows[0]) if part == 0 else (0, key_rows[1], key_rows[2])
                k = jnp.concatenate([k_w[s, b, pl.ds(r, BLK // 2)] for r in blocks], axis=0)
                out[part, b] = lax.dot_general(to_bf16(k), per_head.astype(BF16), NT, preferred_element_type=F32)
        return out

    def softmax(sc):
        p = jnp.exp2(sc - jnp.max(sc, axis=0, keepdims=True))
        total = jnp.sum(p, axis=0, keepdims=True)
        r = pl.reciprocal(total, approx=True)
        return p, r * (2.0 - total * r)

    def weighted_values(s, sc):
        probs = {(0, b): softmax(sc[0, b]) for b in range(B)}
        for b in range(B):
            p, r = softmax(jnp.concatenate([
                sc[1, b][:BLK],
                jnp.where(sees_block_1, sc[1, b][BLK:2 * BLK], -jnp.inf),
                jnp.where(sees_block_2, sc[1, b][2 * BLK:], -jnp.inf)], axis=0))
            probs[1, b] = jnp.concatenate([p[:2 * BLK], jnp.zeros((BLK, 2 * PAIR), F32), p[2 * BLK:]], axis=0), r
        out = {}
        for part in range(2):
            for b in range(B):
                p, r = probs[part, b]
                out[part, b] = []
                for h in range(2):
                    rows = pl.ds(h * BLK // 2, BLK // 2)
                    if part == 0:
                        v = v_w[s, b, 0, rows]
                    else:
                        v = jnp.concatenate([v_w[s, b, 1, rows], v_w[s, b, 2, rows]], axis=1)
                    cols = slice(h * PAIR, (h + 1) * PAIR)
                    pv = jnp.dot(to_bf16(v), p[:, cols].astype(BF16), preferred_element_type=F32)
                    out[part, b].append((pv, r[:, cols]))
        return out

    def store_context(s, heads):
        for part in range(2):
            for b in range(B):
                c = jnp.concatenate([pv * r for pv, r in heads[part, b]], axis=0).astype(BF16).T
                ctx_w[s, pl.ds((2 * b + part) * BLK, BLK)] = pltpu.bitcast(c, I32)

    def project(s, words):
        c = jnp.concatenate([ctx_w[s], ctx_w[s + 1]], axis=1)
        w = jnp.concatenate(
            [jnp.concatenate([w[r:r + BLK] for r in range(0, w.shape[0], BLK)], axis=1) for w in words], axis=0)
        return jnp.dot(to_bf16(c), to_bf16(w), preferred_element_type=F32)

    def received_wq(s):
        return jnp.concatenate([decode(msg.at[s]) for msg in wq_msg], axis=0)

    def received_wo(s, lo, hi, header=None):
        return decode(wo_msg.at[s], range(4 * lo, 4 * hi), header)

    def write_out(row, cols, value):
        for t in range(value.shape[0] // BLK):
            b, place = divmod(row // BLK + t, SQ // BLK)
            out_ref[b, pl.ds(ROW_ORDER[place] * BLK, BLK), cols] = value[t * BLK:(t + 1) * BLK].astype(out_ref.dtype)

    x_load.wait()
    for b in range(B):
        for place, block in enumerate(ROW_ORDER):
            w = to_words(x_f32[b, pl.ds(block * BLK, BLK)] * SCALE)
            for k in range(DM // 128):
                x_w[k, pl.ds((b * SQ + place * BLK) // 2, BLK // 2)] = w[:, k * 128:(k + 1) * 128]
    q = queries(wq_w[0])

    wo_load.wait()
    for h in range(2):
        w = jnp.concatenate(
            [to_words(wo_f32[h * PAIR:(h + 1) * PAIR, j * 128:(j + 1) * 128]) for j in range(DM // 128)], axis=0)
        wo_w[h] = w
        encode(w, wo_msg.at[h])
    for d in range(2):
        start(*wo_copy["first", d][:2])
    k_load[0].wait()
    prepare_keys(0)

    heads = None
    for s in range(SLOTS):
        if s == 1:
            for d in range(2):
                wait_recv(*wq_copy["first", d])
                start(*wq_copy["relay", d], *wo_copy["first", d][2:], *wo_copy["second", d])
        if s == 3:
            for d in range(2):
                wait_recv(*wq_copy["second", d])
        if s == 6:
            for d in range(2):
                wait_recv(*wo_copy["first", d][:2])
                start(*wo_copy["relay", d][:2])
            update = project(2, [received_wo(z, 0, half) for z in (2, 3)])
            store_context(5, heads)
            heads = None
            acc[:, 0:BLK * half] += update
            for d in range(2):
                wait_recv(*wq_copy["relay", d])
            q = queries(received_wq(6))
            for d in range(2):
                wait_recv(*wo_copy["first", d][2:])
                start(*wo_copy["relay", d][2:])
        v_load[s].wait()
        if s + 1 < SLOTS:
            k_load[s + 1].wait()

        sc = scores(s, q)
        if s == 7:
            heads_6 = heads
        elif heads is not None:
            store_context(s - 1, heads)
        if s == 5:
            acc[...] = project(0, (wo_w[0], wo_w[1]))
        elif s == 7:
            acc[:, BLK * half:DM] += project(2, [received_wo(z, half, 8) for z in (2, 3)])
        else:
            q = queries(wq_w[1] if s == 0 else received_wq(s + 1))
        if s + 1 < SLOTS:
            prepare_keys(s + 1)
        prepare_values(s)
        heads = weighted_values(s, sc)

    for d in range(2):
        wait_send(*wq_copy["first", d], *wq_copy["second", d], *wq_copy["relay", d], *wo_copy["first", d])
        wait_recv(*wo_copy["second", d])
    update = project(4, [received_wo(z, 0, 8) for z in (4, 5)])
    for h in range(2):
        store_context(6 + h, {key: [heads_6[key][h], heads[key][h]] for key in heads})
    acc[...] += update

    def finish_output(lo, hi):
        for j in range(lo // 2, (hi + 1) // 2):
            cols = slice(j * 128, (j + 1) * 128)
            hs = [h for h in range(2) if lo <= 2 * j + h < hi]
            w = to_bf16(jnp.concatenate(
                [received_wo(z, 2 * j + h, 2 * j + h + 1, diag_header[z]) for h in hs for z in (6, 7)], axis=0))
            rows = B * SQ * len(hs) // 4
            for r in range(0, B * SQ, rows):
                c = jnp.concatenate([ctx_w[6 + h, pl.ds(r // 2, rows // 2)] for h in hs], axis=1)
                value = acc[pl.ds(r, rows), cols] + jnp.dot(to_bf16(c), w, preferred_element_type=F32)
                if hs[-1] == 0:
                    acc[pl.ds(r, rows), cols] = value
                else:
                    write_out(r, cols, value)

    for i, part in enumerate(WO_PARTS):
        for d in range(2):
            if i == len(WO_PARTS) - 1:
                wait_send(*wo_copy["second", d], *wo_copy["relay", d][:-1])
            wait_recv(*wo_copy["relay", d][(i + 1 if i else 0):i + 2])
        if i == 0:
            diag_header = {z: read_header(wo_msg.at[z]) for z in (6, 7)}
            headers = jnp.zeros((1, 128), I32)
            for s in range(SLOTS):
                for msg in (*wq_msg, wo_msg):
                    headers = headers | msg[s, pl.ds(msg.shape[1] - 8, 1)]
            misfit = jnp.max(jnp.where((headers & MISFIT) != 0, 1.0, 0.0)) > 0.0
        finish_output(*part)
    for d in range(2):
        wait_send(wo_copy["relay", d][-1])

    @pl.when(misfit)
    def _():
        def plain(stage):
            k = 2 * list(ROUTE).index(stage)
            return [remote(buf, stage, d, slice(None), (plain_send_sem, plain_recv_sem), k + i)
                    for d in range(2) for i, buf in enumerate((wq_w, wo_w))]

        for copies in (plain("first") + plain("second"), plain("relay")):
            start(*copies)
            wait_send(*copies)
            wait_recv(*copies)

        def attend(s, carry):
            store_context(s, weighted_values(s, scores(s, queries(wq_w[s]))))
            return carry

        def add(i, carry):
            acc[...] += project(2 * i, (wo_w[2 * i], wo_w[2 * i + 1]))
            return carry

        lax.fori_loop(0, SLOTS, attend, 0)
        acc[...] = jnp.zeros(acc.shape, F32)
        lax.fori_loop(0, SLOTS // 2, add, 0)
        write_out(0, slice(None), acc[...])


def pallas_dist_sparse_attn_blocksparse_qseq_b2_sq256_skv256_hq4_dh64_kernel(
    x: jax.Array,
    Wq: jax.Array,
    K_ext: jax.Array,
    V_ext: jax.Array,
    Wo: jax.Array,
):
    kt = jnp.transpose(K_ext, (0, 2, 3, 1)).reshape(B, SLOTS, PAIR, SKV)
    vt = jnp.transpose(V_ext, (0, 2, 3, 1)).reshape(B, SLOTS, PAIR, SKV)
    return pl.pallas_call(
        _body,
        out_shape=jax.ShapeDtypeStruct((B, SQ, DM), BF16),
        in_specs=[pl.BlockSpec(memory_space=pltpu.HBM)] * 5,
        out_specs=pl.BlockSpec(memory_space=pltpu.VMEM),
        scratch_shapes=[
            pltpu.VMEM((B, SQ, DM), F32),
            pltpu.VMEM((2, DM, PAIR), F32),
            pltpu.VMEM((2 * PAIR, DM), F32),
            pltpu.VMEM((SLOTS, B, PAIR, SKV), F32),
            pltpu.VMEM((SLOTS, B, PAIR, SKV), F32),
            pltpu.VMEM((DM // 128, B * SQ // 2, 128), I32),
            pltpu.VMEM((SLOTS, DM // 2, PAIR), I32),
            pltpu.VMEM((SLOTS, DM // 2, 128), I32),
            pltpu.VMEM((SLOTS, 6 * WQ_GROUPS[0] + 8, 128), I32),
            pltpu.VMEM((SLOTS, 6 * WQ_GROUPS[1] + 8, 128), I32),
            pltpu.VMEM((SLOTS, 6 * 32 + 8, 128), I32),
            pltpu.VMEM((SLOTS, B, SKV // 2, PAIR), I32),
            pltpu.VMEM((SLOTS, B, 3, PAIR // 2, 128), I32),
            pltpu.VMEM((SLOTS, B * SQ // 2, PAIR), I32),
            pltpu.VMEM((B * SQ, DM), F32),
            pltpu.SemaphoreType.DMA((6 + 2 * SLOTS,)),
            pltpu.SemaphoreType.DMA((2, 11 + len(WO_PARTS))),
            pltpu.SemaphoreType.DMA((2, 11 + len(WO_PARTS))),
            pltpu.SemaphoreType.DMA((2, 6)),
            pltpu.SemaphoreType.DMA((2, 6)),
            pltpu.SemaphoreType.REGULAR,
        ],
        compiler_params=pltpu.CompilerParams(
            collective_id=0,
            vmem_limit_bytes=48 * 1024 * 1024,
            disable_bounds_checks=True,
            disable_semaphore_checks=True,
        ),
    )(x, Wq, kt, vt, Wo)
```
